```python
import numpy as np

kernel_name = "dist_sort_i_m128_n64"

def setup_inputs():
    return {"x": np.random.randn(512, 64).astype(np.float32)}

def reference(x: np.ndarray) -> np.ndarray:
    return np.sort(x, axis=0)
```

```python
import numpy as np

import jax
import jax.numpy as jnp
from jax import lax
from jax.experimental import pallas as pl
from jax.experimental.pallas import tpu as pltpu

SUB, LANES = 8, 128
ROWS, COLS = 128, 64
HALF = COLS // 2

_SORT16 = (
    ((0, 1), (2, 3), (4, 5), (6, 7), (8, 9), (10, 11), (12, 13), (14, 15)),
    ((0, 2), (1, 3), (4, 6), (5, 7), (8, 10), (9, 11), (12, 14), (13, 15)),
    ((0, 4), (1, 5), (2, 6), (3, 7), (8, 12), (9, 13), (10, 14), (11, 15)),
    ((0, 8), (1, 9), (2, 10), (3, 11), (4, 12), (5, 13), (6, 14), (7, 15)),
    ((1, 2), (3, 12), (4, 8), (5, 10), (6, 9), (7, 11), (13, 14)),
    ((1, 4), (2, 8), (5, 6), (7, 13), (9, 10), (11, 14)),
    ((2, 4), (3, 8), (7, 12), (11, 13)),
    ((3, 5), (6, 8), (7, 9), (10, 12)),
    ((3, 4), (5, 6), (7, 8), (9, 10), (11, 12)),
    ((6, 7), (8, 9)),
)


class _Consts:
    def __init__(self):
        self.sub = lax.broadcasted_iota(jnp.int32, (SUB, LANES), 0)
        self.lane = lax.broadcasted_iota(jnp.int32, (SUB, LANES), 1)
        self._memo = {}

    def _get(self, key, make):
        if key not in self._memo:
            self._memo[key] = make()
        return self._memo[key]

    def sub_table(self, table):
        table = tuple(int(t) for t in table)
        if all(t == s ^ table[0] for s, t in enumerate(table)):
            return self._get(("xor", table[0]), lambda: self.sub ^ table[0])
        word = sum(t << (4 * s) for s, t in enumerate(table))
        return self._get(
            ("tab", word), lambda: lax.shift_right_logical(word, self.sub << 2) & 7
        )

    def sub_mask(self, flags):
        word = sum(int(bool(f)) << s for s, f in enumerate(flags))
        return self._get(
            ("msk", word), lambda: (lax.shift_right_logical(word, self.sub) & 1) == 1
        )

    def lane_bit(self, bit):
        return self._get(("lane", bit), lambda: (self.lane & (1 << bit)) != 0)


def _shuffle(x, idx):
    return jnp.take_along_axis(x, idx, axis=0, mode="promise_in_bounds")


class _Seq:
    def __init__(self, k, tiles, pos):
        self.k = k
        self.tiles = list(tiles)
        self.pos = [np.asarray(p) for p in pos]

    def _owner(self, wanted):
        for v, p in enumerate(self.pos):
            if set(p) == set(wanted):
                return v
        raise AssertionError("elements are not in a single tile")

    def _aligned(self, tile, have, wanted):
        if (have == wanted).all():
            return tile
        table = [int(np.nonzero(have == w)[0][0]) for w in wanted]
        return _shuffle(tile, self.k.sub_table(table))

    def fetch(self, wanted):
        out = None
        for tile, have in zip(self.tiles, self.pos):
            hit = np.isin(wanted, have)
            if not hit.any():
                continue
            table = [
                int(np.nonzero(have == w)[0][0]) if h else s
                for s, (w, h) in enumerate(zip(wanted, hit))
            ]
            if table != list(range(SUB)):
                tile = _shuffle(tile, self.k.sub_table(table))
            out = tile if out is None else jnp.where(self.k.sub_mask(hit), tile, out)
        return out

    def pairs(self, mask, evict):
        done, out = set(), []
        for v, p in enumerate(self.pos):
            if v in done:
                continue
            w = self._owner(p ^ mask)
            if w != v:
                if evict is not None and (p[0] >> evict) & 1 and mask >> evict & 1:
                    continue
                a, pa = self.tiles[v], p
                b = self._aligned(self.tiles[w], self.pos[w], p ^ mask)
            else:
                if (p[0] >> evict) & 1:
                    continue
                w = self._owner(p ^ (1 << evict))
                assert w != v
                q = p ^ (1 << evict)
                other = self._aligned(self.tiles[w], self.pos[w], q)
                first = np.array(
                    [s < int(np.nonzero(p == (i ^ mask))[0][0]) for s, i in enumerate(p)]
                )
                m = self.k.sub_mask(first)
                a, pa = jnp.where(m, self.tiles[v], other), np.where(first, p, q)
                b = self._aligned(
                    jnp.where(m, other, self.tiles[v]), np.where(first, q, p), pa ^ mask
                )
            done.update((v, w))
            out.append((a, b, np.minimum(pa, pa ^ mask), np.maximum(pa, pa ^ mask)))
        assert len(done) == len(self.pos)
        return out

    def exchange(self, mask, evict=None):
        tiles, pos = [], []
        for a, b, lo, hi in self.pairs(mask, evict):
            tiles += [jnp.minimum(a, b), jnp.maximum(a, b)]
            pos += [lo, hi]
        order = sorted(range(len(pos)), key=lambda v: pos[v].min())
        return _Seq(self.k, [tiles[v] for v in order], [pos[v] for v in order])

    def exchange_pick(self, bit, upper, evict=None):
        tiles, pos = [], []
        for a, b, lo, _ in self.pairs(1 << bit, evict):
            tiles.append(jnp.where(upper, jnp.maximum(a, b), jnp.minimum(a, b)))
            pos.append(lo)
        return _Seq(self.k, tiles, pos)

    def exchange_in_tile(self, bit):
        tiles = []
        for a, p in zip(self.tiles, self.pos):
            b = self._aligned(a, p, p ^ (1 << bit))
            upper = self.k.sub_mask((p >> bit) & 1)
            tiles.append(jnp.where(upper, jnp.maximum(a, b), jnp.minimum(a, b)))
        return _Seq(self.k, tiles, self.pos)


def _rotate_tiles(tiles, amount):
    n = len(tiles)
    step = 1
    while step < n:
        m = (amount & step) != 0
        tiles = [jnp.where(m, tiles[(j + step) % n], tiles[j]) for j in range(n)]
        step *= 2
    return tiles


def _columns_to_lanes(k, tiles):
    t = k.sub + k.lane
    skew = _rotate_tiles([_shuffle(x, t & 7) for x in tiles], t >> 3)
    return [
        pltpu.roll(skew[j % len(tiles)], SUB * j, 1, stride=1, stride_axis=0)
        for j in range(ROWS // SUB)
    ]


def _sort_up_to_last_bits(k, tiles):
    tiles = list(tiles)
    for layer in _SORT16:
        for i, j in layer:
            tiles[i], tiles[j] = (
                jnp.minimum(tiles[i], tiles[j]),
                jnp.maximum(tiles[i], tiles[j]),
            )
    q = _Seq(k, tiles, [v + 16 * np.arange(SUB) for v in range(16)])
    for mask, evict in (
        (31, 0), (8, None), (4, None), (2, None), (1, 1),
        (63, 0), (16, None), (8, None), (4, None), (2, 2), (1, 1),
        (127, 0), (32, None), (16, None), (8, None), (4, 3),
    ):
        q = q.exchange(mask, evict)
    return q


def _sort(k, tiles):
    return _sort_up_to_last_bits(k, tiles).exchange(2, 2).exchange(1, 1)


_PLAIN = [SUB * v + np.arange(SUB) for v in range(ROWS // SUB)]


def _relayout(q, pos):
    return _Seq(q.k, [q.fetch(p) for p in pos], pos)


def _clean(q):
    for bit in (6, 5, 4, 3):
        q = q.exchange(1 << bit)
    for bit in (2, 1, 0):
        q = q.exchange_in_tile(bit)
    return q


def _against(op, a, b):
    return _Seq(a.k, [op(x, b.fetch(127 - p)) for x, p in zip(a.tiles, a.pos)], a.pos)


def _tile(ref, j):
    return ref[pl.ds(SUB * j, SUB), :]


def _store_bf16(ref, tiles):
    for j in range(0, len(tiles), 2):
        pair = jnp.concatenate(tiles[j : j + 2], axis=0)
        ref[pl.ds(SUB * j, 2 * SUB), :] = pair.astype(jnp.bfloat16)


def _load_bf16(ref):
    tiles = []
    for j in range(0, ref.shape[0] // SUB, 2):
        pair = ref[pl.ds(SUB * j, 2 * SUB), :].astype(jnp.float32)
        tiles += [pair[:SUB], pair[SUB:]]
    return tiles


def _store_list(k, ref, q):
    upper = k.lane_bit(6)
    _store_bf16(ref, [jnp.where(upper, q.tiles[j + 8], q.tiles[j]) for j in range(8)])


def _load_list(k, ref):
    upper = k.lane_bit(6)
    here = _load_bf16(ref)
    moved = [pltpu.roll(x, COLS, 1) for x in here]
    lo = [jnp.where(upper, m, x) for x, m in zip(here, moved)]
    hi = [jnp.where(upper, x, m) for x, m in zip(here, moved)]
    return _Seq(k, lo + hi, _PLAIN)


def _emit_replicated(k, q, o_ref, n_tiles):
    t = k.sub + k.lane
    tiles = q.tiles
    skew = _rotate_tiles([_shuffle(x, t & 7) for x in tiles], t >> 3)
    moved = [
        pltpu.roll(skew[j], SUB * j, 1, stride=1, stride_axis=0) for j in range(n_tiles)
    ]
    d = k.lane - k.sub
    back = [_shuffle(x, d & 7) for x in moved]
    back = _rotate_tiles([back[-j % n_tiles] for j in range(n_tiles)], -(d >> 3))
    for j in range(n_tiles):
        o_ref[pl.ds(SUB * j, SUB), :] = back[j]


def _emit_interleaved(k, q, o_ref, first_tile):
    where = {int(i) >> 2: (u, s) for u, p in enumerate(q.pos) for s, i in enumerate(p)}
    assert all(where[r][0] == r >> 3 and where[r][1] == where[r & 7][1] for r in where)
    word = sum(where[r][1] << (4 * r) for r in range(SUB))
    plain = all(where[r][1] == r for r in range(SUB))
    done = []
    for a in range(4):
        t = ((k.lane + a) >> 2) + k.sub
        idx = t & 7
        if not plain:
            idx = lax.shift_right_logical(word, idx << 2) & 7
        skew = _rotate_tiles([_shuffle(x, idx) for x in q.tiles], t >> 3)
        g = [
            pltpu.roll(skew[j], 32 * j + a, 1, stride=4, stride_axis=0) for j in range(4)
        ]
        g = [
            jnp.where(k.lane_bit(1), jnp.maximum(x, y), jnp.minimum(x, y))
            for x, y in ((g[0], g[2]), (g[1], g[3]))
        ]
        done.append(
            jnp.where(k.lane_bit(0), jnp.maximum(g[0], g[1]), jnp.minimum(g[0], g[1]))
        )
    d = k.lane - k.sub
    for j in range(4):
        idx = ((d >> 2) - 2 * j) & 7
        out = _shuffle(done[0], idx)
        for a in range(1, 4):
            out = jnp.where((d & 3) == a, _shuffle(done[a], idx), out)
        o_ref[pl.ds(SUB * (first_tile + j), SUB), :] = out


def _body(x_hbm, o_ref, x_ref, raw_ref, fast_ref, mine_ref, lists_ref,
          load_sem, fast_sem, send_sem, recv_sem, go_sem):
    me = lax.axis_index("i")
    barrier = pltpu.get_barrier_semaphore()
    logical = pl.DeviceIdType.LOGICAL
    head, tail = pl.ds(0, HALF), pl.ds(HALF, HALF)
    load_tail = pltpu.make_async_copy(x_hbm.at[tail], x_ref.at[tail], load_sem.at[0])
    load_head = pltpu.make_async_copy(x_hbm.at[head], x_ref.at[head], load_sem.at[1])
    raw = pltpu.make_async_remote_copy(
        x_hbm.at[head], raw_ref, fast_sem.at[0], fast_sem.at[1],
        device_id=0, device_id_type=logical,
    )
    fast = pltpu.make_async_remote_copy(
        fast_ref, fast_ref, fast_sem.at[2], fast_sem.at[3],
        device_id=0, device_id_type=logical,
    )

    def send(step):
        return pltpu.make_async_remote_copy(
            mine_ref, lists_ref.at[step - 1], send_sem.at[step - 1],
            recv_sem.at[step - 1], device_id=me ^ step, device_id_type=logical,
        )

    def signal(sem, chip):
        pl.semaphore_signal(sem, 1, device_id=chip, device_id_type=logical)

    fast_pos = []
    load_tail.start()

    @pl.when(me == 2)
    def _():
        k = _Consts()
        pl.semaphore_wait(barrier, 3)
        raw.start()
        for chip in (1, 3, 0):
            signal(go_sem, chip)
        load_head.start()
        load_tail.wait()
        q = _sort_up_to_last_bits(
            k, _columns_to_lanes(k, [_tile(x_ref, 4 + j) for j in range(4)])
        )
        q = q.exchange_pick(1, ~k.lane_bit(6), 2).exchange_pick(0, ~k.lane_bit(5), 4)
        fast_pos.extend(q.pos)
        _store_bf16(fast_ref, q.tiles)
        fast.start()

    @pl.when(me != 2)
    def _():
        signal(barrier, 2)

        @pl.when(me == 0)
        def _():
            signal(barrier, 1)
            signal(barrier, 3)

        load_head.start()
        load_tail.wait()

    load_head.wait()
    k = _Consts()
    mine = _relayout(
        _sort(k, _columns_to_lanes(k, [_tile(x_ref, j) for j in range(8)])), _PLAIN
    )
    _store_list(k, mine_ref, mine)

    @pl.when(me == 0)
    def _():
        k = _Consts()
        pl.semaphore_wait(go_sem, 1)
        for step in (2, 1, 3):
            send(step).start()
        w = _Seq(k, mine.tiles, mine.pos)
        for step in (1, 3):
            send(step).wait_recv()
            w = _clean(_against(jnp.minimum, w, _load_list(k, lists_ref.at[step - 1])))
        moved = [pltpu.roll(x, HALF, 1) for x in w.tiles]
        odd = k.lane_bit(5)
        w_head = _Seq(k, [jnp.where(odd, m, x) for x, m in zip(w.tiles, moved)], w.pos)
        w_tail = _Seq(k, [jnp.where(odd, x, m) for x, m in zip(w.tiles, moved)], w.pos)
        w_fast = []
        for p in fast_pos:
            b = [w_tail.fetch(127 - p - 3 + i) for i in range(4)]
            w_fast.append(
                jnp.where(
                    k.lane_bit(6), jnp.where(odd, b[3], b[2]), jnp.where(odd, b[1], b[0])
                )
            )

        raw.wait_recv()
        q = _sort(k, _columns_to_lanes(k, [_tile(raw_ref, j) for j in range(4)]))
        q = _clean(_against(jnp.minimum, w_head, q))
        _emit_replicated(k, q, o_ref, 4)

        fast.wait_recv()
        got = _load_bf16(fast_ref)
        q = _Seq(
            k,
            [jnp.minimum(x, y) for x, y in zip(got, w_fast)],
            [124 - p for p in fast_pos],
        )
        q = q.exchange(64).exchange(32)
        for bit in (4, 3, 2):
            q = q.exchange_in_tile(bit)
        _emit_interleaved(k, q, o_ref, 4)
        for step in (2, 1, 3):
            send(step).wait_send()

    @pl.when(me != 0)
    def _():
        k = _Consts()

        @pl.when(me == 2)
        def _():
            for step in (1, 3):
                send(step).start()
            raw.wait_send()
            fast.wait_send()

        @pl.when(me != 2)
        def _():
            pl.semaphore_wait(barrier, 1)
            send(me).start()
            pl.semaphore_wait(go_sem, 1)
            send(2).start()
            send(me ^ 2).start()
            send(2).wait_send()

        for step in (1, 3):
            send(step).wait_send()
        for step in (1, 3, 2):
            send(step).wait_recv()
        a = _Seq(k, mine.tiles, mine.pos)
        b, c, d = (_load_list(k, lists_ref.at[i]) for i in range(3))
        lo1, hi1 = (_clean(_against(op, a, b)) for op in (jnp.minimum, jnp.maximum))
        lo2, hi2 = (_clean(_against(op, c, d)) for op in (jnp.minimum, jnp.maximum))

        def pick(upper):
            return lambda x, y: jnp.where(upper, jnp.maximum(x, y), jnp.minimum(x, y))

        first = _against(pick(me >= 2), lo1, hi2)
        second = _against(pick(me >= 2), hi1, lo2)
        q = _Seq(
            k,
            [pick((me & 1) == 1)(x, y) for x, y in zip(first.tiles, second.tiles)],
            _PLAIN,
        )
        _emit_replicated(k, _clean(q), o_ref, 8)


def pallas_dist_sort_i_m128_n64_kernel(x: jax.Array):
    xt = x.T
    out = pl.pallas_call(
        _body,
        out_shape=jax.ShapeDtypeStruct(xt.shape, xt.dtype),
        in_specs=[pl.BlockSpec(memory_space=pltpu.MemorySpace.HBM)],
        out_specs=pl.BlockSpec(memory_space=pltpu.VMEM),
        scratch_shapes=[
            pltpu.VMEM((COLS, ROWS), jnp.float32),
            pltpu.VMEM((HALF, ROWS), jnp.float32),
            pltpu.VMEM((4 * SUB, LANES), jnp.bfloat16),
            pltpu.VMEM((8 * SUB, LANES), jnp.bfloat16),
            pltpu.VMEM((3, 8 * SUB, LANES), jnp.bfloat16),
            pltpu.SemaphoreType.DMA((2,)),
            pltpu.SemaphoreType.DMA((4,)),
            pltpu.SemaphoreType.DMA((3,)),
            pltpu.SemaphoreType.DMA((3,)),
            pltpu.SemaphoreType.REGULAR,
        ],
        compiler_params=pltpu.CompilerParams(
            collective_id=0,
            disable_bounds_checks=True,
            disable_semaphore_checks=True,
        ),
    )(xt)
    return out.T
```

```python
import jax
import jax.numpy as jnp
import numpy as np
from jax import lax
from jax.experimental import pallas as pl
from jax.experimental.pallas import tpu as pltpu

SUB, LANES = 8, 128
COLS = 64

_MERGES_128 = (
    (31, 0), (8, None), (4, None), (2, None), (1, 1),
    (63, 0), (16, None), (8, None), (4, None), (2, 2), (1, 1),
    (127, 0), (32, None), (16, None), (8, None), (4, 3), (2, 2), (1, 1),
)
_MERGES_64 = (
    (15, 0), (4, None), (2, None), (1, 1),
    (31, 0), (8, None), (4, None), (2, 2), (1, 1),
    (63, 0), (16, None), (8, None), (4, 3), (2, 2), (1, 1),
)
_CLEAN_128 = ((64, None), (32, None), (16, None), (8, 0), (4, 3), (2, 2), (1, 1))
_CLEAN_64 = _CLEAN_128[1:]


class _Consts:
    def __init__(self):
        self.sub = lax.broadcasted_iota(jnp.int32, (SUB, LANES), 0)
        self.lane = lax.broadcasted_iota(jnp.int32, (SUB, LANES), 1)
        self.makers = {}
        self.values = {}

    def get(self, key, make, *args):
        key = (key, *args)
        if key not in self.values:
            self.makers[key] = make
            self.values[key] = make(self.sub, self.lane, *args)
        return self.values[key]

    def prepare(self, fn, n_tiles):
        makers = {}

        def record():
            k = _Consts()
            fn(k, [jnp.zeros((SUB, LANES), jnp.float32)] * n_tiles)
            makers.update(k.makers)

        jax.eval_shape(record)
        for (key, *args), make in makers.items():
            self.get(key, make, *args)

    def sub_table(self, table):
        if all(t == s ^ table[0] for s, t in enumerate(table)):
            return self.get("xor", lambda s, l, x: s ^ x, table[0])
        word = sum(t << (4 * s) for s, t in enumerate(table))
        return self.get("table", lambda s, l, x: (x >> (s << 2)) & 7, word)

    def sub_mask(self, flags):
        word = sum(int(f) << s for s, f in enumerate(flags))
        return self.get("mask", lambda s, l, x: ((x >> s) & 1) == 1, word)

    def lane_bit(self, bit):
        return self.get("lane", lambda s, l, x: (l & x) != 0, 1 << bit)


def _take(x, idx, axis):
    numbers = lax.GatherDimensionNumbers(
        offset_dims=(),
        collapsed_slice_dims=(axis,),
        start_index_map=(axis,),
        operand_batching_dims=(1 - axis,),
        start_indices_batching_dims=(1 - axis,),
    )
    mode = lax.GatherScatterMode.PROMISE_IN_BOUNDS
    return lax.gather(x, idx[..., None], numbers, (1, 1), mode=mode)


def _pick(upper, a, b):
    return jnp.where(upper, jnp.maximum(a, b), jnp.minimum(a, b))


def _swap(flip, a, b):
    return jnp.where(flip, b, a), jnp.where(flip, a, b)


class _Seq:
    def __init__(self, k, tiles, pos, descending=False):
        self.k = k
        self.tiles = list(tiles)
        self.pos = list(pos)
        self.descending = descending

    def _tile_of(self, wanted):
        (v,) = [v for v, p in enumerate(self.pos) if sorted(p) == sorted(wanted)]
        return v

    def _aligned(self, tile, have, wanted):
        table = [list(have).index(w) if w in have else s for s, w in enumerate(wanted)]
        if table == list(range(SUB)):
            return tile
        return _take(tile, self.k.sub_table(table), 0)

    def fetch(self, wanted):
        out = None
        for tile, have in zip(self.tiles, self.pos):
            hit = np.isin(wanted, have)
            if hit.any():
                tile = self._aligned(tile, have, wanted)
                out = tile if out is None else jnp.where(self.k.sub_mask(hit), tile, out)
        return out

    def pairs(self, mask, evict):
        done, out = [], []
        for v, p in enumerate(self.pos):
            w = self._tile_of(p ^ mask)
            if v in done or (evict is not None and p[0] >> evict & 1):
                continue
            if w == v:
                q = p ^ (1 << evict)
                w = self._tile_of(q)
                later = np.array([list(p).index(i ^ mask) < s for s, i in enumerate(p)])
                a, b = _swap(self.k.sub_mask(later), self.tiles[v], self.fetch(q))
                p, q = np.where(later, q, p), np.where(later, p, q)
                b = self._aligned(b, q, p ^ mask)
            else:
                a, b = self.tiles[v], self.fetch(p ^ mask)
            done += [v, w]
            out.append((a, b, np.minimum(p, p ^ mask), np.maximum(p, p ^ mask)))
        assert sorted(done) == list(range(len(self.pos)))
        return out

    def exchange(self, stages):
        q = self
        for mask, evict in stages:
            tiles, pos = [], []
            for a, b, lo, hi in q.pairs(mask, evict):
                tiles += [jnp.minimum(a, b), jnp.maximum(a, b)]
                pos += [hi, lo] if q.descending else [lo, hi]
            order = sorted(range(len(pos)), key=lambda v: pos[v].min())
            tiles, pos = [tiles[v] for v in order], [pos[v] for v in order]
            q = _Seq(q.k, tiles, pos, q.descending)
        return q

    def exchange_pick(self, bit, upper, evict=None):
        pairs = self.pairs(1 << bit, evict)
        tiles = [_pick(upper, a, b) for a, b, _, _ in pairs]
        return _Seq(self.k, tiles, [lo for _, _, lo, _ in pairs])

    def against(self, op, other):
        tiles = [op(x, other.fetch(127 - p)) for x, p in zip(self.tiles, self.pos)]
        return _Seq(self.k, tiles, self.pos)

    def window(self, below, above):
        tiles = [jnp.minimum(x, y) for x, y in zip(self.tiles, above)]
        if below is not None:
            tiles = [jnp.maximum(x, y) for x, y in zip(tiles, below)]
        return _Seq(self.k, tiles, self.pos).exchange(_CLEAN_64)

    def sublane_bits(self):
        bits = [int(self.pos[0][1 << b]) for b in range(3)]
        spread = [sum(x for b, x in enumerate(bits) if s >> b & 1) for s in range(SUB)]
        assert all(list(p & sum(bits)) == spread for p in self.pos)
        return bits


def _sublane_of(index, bits):
    return sum(jnp.where((index & x) != 0, 1 << b, 0) for b, x in enumerate(bits))


def _merge_tiles(a, b):
    if not a or not b:
        return a + b
    if len(a) + len(b) == 2:
        return [jnp.minimum(*a, *b), jnp.maximum(*a, *b)]
    even, odd = _merge_tiles(a[::2], b[::2]), _merge_tiles(a[1::2], b[1::2])
    out = even[:1]
    for x, y in zip(odd, even[1:]):
        out += _merge_tiles([x], [y])
    return out + odd[len(even) - 1 :] + even[len(odd) + 1 :]


def _sort_tiles(tiles):
    half = len(tiles) // 2
    if not half:
        return tiles
    return _merge_tiles(_sort_tiles(tiles[:half]), _sort_tiles(tiles[half:]))


def _runs(k, tiles, descending=False, order=tuple(range(SUB))):
    pos = [v + len(tiles) * np.array(order) for v in range(len(tiles))]
    return _Seq(k, tiles[::-1] if descending else tiles, pos, descending)


def _sort_128(k, tiles):
    return _runs(k, _sort_tiles(tiles)).exchange(_MERGES_128)


def _halves(k, tiles):
    odd = k.lane_bit(0)[: tiles[0].shape[0]]
    return list(zip(*(_swap(odd, a, b) for a, b in zip(tiles[::2], tiles[1::2]))))


def _half_to_lanes(k, tiles, p):
    idx = k.get("in", lambda s, l, p: (s + ((l + p) >> 1)) & 7, p)
    skew = [_take(x, idx, 0) for x in tiles]
    n, step = len(tiles), 1
    while step < n:
        m = k.get("in", lambda s, l, p, x: ((s + ((l + p) >> 1)) & x) != 0, p, 8 * step)
        skew = [jnp.where(m, skew[(j + step) % n], skew[j]) for j in range(n)]
        step *= 2
    return [
        pltpu.roll(skew[j % n], 16 * j + p, 1, stride=2, stride_axis=0)
        for j in range(8)
    ]


def _columns_to_lanes(k, tiles):
    return [x for p, h in enumerate(_halves(k, tiles)) for x in _half_to_lanes(k, h, p)]


def _presort(k, tiles):
    x = _columns_to_lanes(k, tiles)
    done = []
    for group in ((4, 5, 10, 0, 2, 11, 1, 3), (15, 6, 8, 7), (9, 12, 14, 13)):
        done = _merge_tiles(done, _sort_tiles([x[i] for i in group]))
    q = _runs(k, done).exchange(_MERGES_128[:12])
    for h in (slice(0, 8), slice(8, 16)):
        r = _Seq(k, q.tiles[h], q.pos[h]).exchange(_MERGES_128[12:15])
        for bit in (2, 1, 0):
            r = r.exchange_pick(bit, k.lane_bit(4 + bit), 5 - bit)
        yield r


def _blocks_to_rows(q, groups):
    k = q.k
    bits = q.sublane_bits()
    assert [int(p[0]) for p in q.pos] == [0, 1, 16, 17, 32, 33, 48, 49]
    x = [lax.bitcast_convert_type(t, jnp.int32) for t in q.tiles]
    x = [hi | lax.shift_right_logical(lo, 16) for lo, hi in zip(x[:4], x[4:])]
    idx = k.get("out", lambda s, l: s ^ ((l >> 1) & 7))
    x = [_take(t, idx, 0) for t in x]
    first, second = _swap(k.lane_bit(0), *x[:2]), _swap(k.lane_bit(0), *x[2:])
    back = k.get("back", lambda s, l, *bits: s ^ _sublane_of(l, bits), *bits)

    def source(s, l, g, g_next, b, *bits):
        group = jnp.where((l & 16) != 0, 16 * g_next, 16 * g)
        return group | ((l & 65) ^ b) | ((s ^ _sublane_of(l, bits)) << 1)

    moved = []
    for g in range(groups):
        here = k.get("group", lambda s, l, g: ((l >> 4) & 3) == g, g)
        x = [
            _take(
                jnp.where(here, first[b], second[b]),
                k.get("source", source, g, (g + 1) % groups, b, *bits),
                1,
            )
            for b in range(2)
        ]
        moved.append(_swap(k.lane_bit(0), *(_take(t, back, 0) for t in x)))
    x = [
        jnp.where(k.lane_bit(4), moved[g - 1][b], moved[g][b])
        for g in range(groups)
        for b in range(2)
    ]
    x = [jnp.where(k.lane_bit(5), t & -65536, t << 16) for t in x]
    return [lax.bitcast_convert_type(t, jnp.float32) for t in x]


def _spread(q, shifts):
    k = q.k
    bits = q.sublane_bits()
    assert [int(p[0]) for p in q.pos] == [0, 8]
    flip = k.get("flip", lambda s, l: ((l + s) & 8) != 0)
    index = lambda s, l, i, *bits: _sublane_of(l + s + i, bits)
    moved = []
    for e in shifts:
        x = [
            _take(t, k.get("spread", index, i, *bits), 0)
            for t, i in zip(q.tiles, (e + 8, e))
        ]
        moved += [
            pltpu.roll(t, e + 8 * a, 1, stride=1, stride_axis=0)
            for a, t in enumerate(_swap(flip, *x))
        ]
    return moved


def _spread_to_rows(k, moved):
    for bit in (2, 1, 0):
        n = len(moved) // 2
        moved = [_pick(k.lane_bit(bit), x, y) for x, y in zip(moved[:n], moved[n:])]
    rows = []
    for b in range(2):
        at = k.lane - 2 * k.sub - b
        lo, hi = (_take(x, at & 7, 0) for x in moved)
        rows.append(jnp.where((at & 8) != 0, hi, lo))
    return rows


def _positions(fn, n_tiles):
    pos = []

    def record():
        for q in fn(_Consts(), [jnp.zeros((SUB, LANES), jnp.float32)] * n_tiles):
            pos.extend(q.pos)

    jax.eval_shape(record)
    return pos


def _tile(ref, j):
    return ref[pl.ds(SUB * j, SUB), :]


def _store(ref, first, tiles):
    for j, x in enumerate(tiles):
        ref[pl.ds(SUB * (first + j), SUB), :] = x


def _store_bf16(ref, tiles):
    for j in range(0, len(tiles), 2):
        pair = jnp.concatenate(tiles[j : j + 2], axis=0)
        ref[pl.ds(SUB * j, 2 * SUB), :] = pair.astype(jnp.bfloat16)


def _load_bf16(ref):
    tiles = []
    for j in range(0, ref.shape[0] // SUB, 2):
        pair = ref[pl.ds(SUB * j, 2 * SUB), :].astype(jnp.float32)
        tiles += [pair[:SUB], pair[SUB:]]
    return tiles


def _rounded(x):
    return x.astype(jnp.bfloat16).astype(jnp.float32)


def _to_words(x):
    return pltpu.bitcast(x.astype(jnp.bfloat16), jnp.uint32)


def _from_words(x):
    x = pltpu.bitcast(x, jnp.bfloat16).astype(jnp.float32)
    return [x[:SUB], x[SUB:]]


def _kernel(x_hbm, o_ref, x_ref, raw_ref, half_ref, sorted_ref, side_raw, side_ref,
            mine_ref, lists_ref, load_sem, first_send, first_recv, send_sem,
            recv_sem, go_sem):
    me = lax.axis_index("i")
    barrier = pltpu.get_barrier_semaphore()
    logical = pl.DeviceIdType.LOGICAL
    loads = [
        pltpu.make_async_copy(x_hbm.at[rows], x_ref.at[rows], load_sem.at[n])
        for n, rows in enumerate(
            (pl.ds(16, 12), pl.ds(0, 16), pl.ds(48, 16), pl.ds(28, 20))
        )
    ]

    def to_first(n, src, dst):
        return pltpu.make_async_remote_copy(
            src, dst, first_send.at[n], first_recv.at[n],
            device_id=0, device_id_type=logical,
        )

    raw = [
        to_first(n, x_hbm.at[pl.ds(16 + at, count)], raw_ref.at[pl.ds(at, count)])
        for n, (at, count) in enumerate(((12, 20), (4, 4)))
    ]
    half = [
        to_first(2 + n, half_ref.at[p, rows], half_ref.at[p, rows])
        for n, (p, rows) in enumerate(
            ((0, pl.ds(4, 2)), (0, pl.ds(0, 4)), (1, pl.ds(0, 6)))
        )
    ]
    presorted = [
        to_first(5 + n, sorted_ref.at[rows], sorted_ref.at[rows])
        for n, rows in enumerate((pl.ds(0, 4), pl.ds(4, 4)))
    ]

    def side(n):
        return (
            to_first(7 + n, x_hbm.at[pl.ds(16, 32)], side_raw.at[n]),
            to_first(9 + n, side_ref.at[n], side_ref.at[n]),
        )

    def send(n, chip, slot):
        return pltpu.make_async_remote_copy(
            mine_ref, lists_ref.at[slot], send_sem.at[n], recv_sem.at[slot],
            device_id=chip, device_id_type=logical,
        )

    def signal(sem, chip, count=1):
        pl.semaphore_signal(sem, count, device_id=chip, device_id_type=logical)

    loads[0].start()

    @pl.when(me == 2)
    def _():
        pl.semaphore_wait(barrier, 2)
        raw[0].start()

    loads[1].start()
    loads[2].start()

    @pl.when(me == 2)
    def _():
        raw[1].start()
        signal(go_sem.at[1], 0)
        k = _Consts()
        k.prepare(lambda k, x: list(_presort(k, x)), 2)
        loads[0].wait()
        x = [x_ref[pl.ds(16, 4), :], x_ref[pl.ds(24, 4), :]]
        for p, (x,) in enumerate(_halves(k, x)):
            half_ref[p, pl.ds(4, 2), :] = _to_words(x)
        half[0].start()
        loads[1].wait()
        for p, (x,) in enumerate(_halves(k, [_tile(x_ref, 0), _tile(x_ref, 1)])):
            half_ref[p, pl.ds(0, 4), :] = _to_words(x)
        half[1].start()
        half[2].start()
        loads[2].wait()
        for n, q in enumerate(_presort(k, [_tile(x_ref, 6), _tile(x_ref, 7)])):
            sorted_ref[pl.ds(4 * n, 4), :] = _to_words(*q.tiles)
            presorted[n].start()
        loads[3].start()

    @pl.when(me == 0)
    def _():
        signal(barrier, 2, 2)
        signal(barrier, 1)
        signal(barrier, 3)
        loads[3].start()
        for load in loads[:3]:
            load.wait()

    @pl.when((me & 1) == 1)
    def _():
        signal(barrier, 0)
        pl.semaphore_wait(barrier, 1)
        copies = side(me >> 1)
        copies[0].start()
        loads[3].start()
        for load in loads[:3]:
            load.wait()
        _store_bf16(side_ref.at[me >> 1], [_tile(x_ref, j) for j in (0, 1, 6, 7)])
        copies[1].start()

    loads[3].wait()
    k = _Consts()
    mine = _columns_to_lanes(k, [_rounded(_tile(x_ref, j)) for j in range(8)])
    mine = _sort_128(k, mine)
    _store_bf16(
        mine_ref,
        [jnp.where(k.lane_bit(6), b, a) for a, b in zip(mine.tiles, mine.tiles[8:])],
    )

    @pl.when(me != 0)
    def _():
        @pl.when(me == 2)
        def _():
            pl.semaphore_wait(barrier, 1)
            signal(go_sem.at[1], 1)
            signal(go_sem.at[1], 3)
            send(0, 1, 2).start()
            send(1, 3, 2).start()
            for copy in (*raw, *half, *presorted):
                copy.wait_send()

        @pl.when(me != 2)
        def _():
            pl.semaphore_wait(go_sem.at[0], 1)
            send(0, me ^ 2, 1).start()
            pl.semaphore_wait(go_sem.at[1], 1)
            send(1, 2, (me + 1) >> 1).start()
            for copy in side(me >> 1):
                copy.wait_send()

        k = _Consts()

        def received(slot):
            tiles = [
                _swap(k.lane_bit(6), x, pltpu.roll(x, COLS, 1))
                for x in _load_bf16(lists_ref.at[slot])
            ]
            return _Seq(k, [x[h] for h in range(2) for x in tiles], mine.pos)

        def merged(a, b):
            ops = (jnp.minimum, jnp.maximum)
            return [a.against(op, b).exchange(_CLEAN_128) for op in ops]

        send(0, 0, 0).wait_recv()
        lo1, hi1 = merged(_Seq(k, mine.tiles, mine.pos), received(0))
        send(0, 0, 1).wait_recv()
        send(0, 0, 2).wait_recv()
        lo2, hi2 = merged(received(1), received(2))
        a = lo1.against(lambda x, y: _pick(me >= 2, x, y), hi2)
        b = hi1.against(lambda x, y: _pick(me >= 2, x, y), lo2)
        q = [_pick((me & 1) == 1, x, y) for x, y in zip(a.tiles, b.tiles)]
        q = _Seq(k, q, a.pos).exchange_pick(6, k.lane_bit(6)).exchange(_CLEAN_64)
        _store(o_ref, 0, _blocks_to_rows(q, 4))
        send(0, 0, 0).wait_send()
        send(1, 0, 0).wait_send()

    @pl.when(me == 0)
    def _():
        k = _Consts()
        pl.semaphore_wait(barrier, 2)
        signal(go_sem.at[0], 1)
        signal(go_sem.at[0], 3)
        signal(barrier, 2)
        send(0, 1, 0).start()
        send(1, 3, 0).start()

        sides = []
        for n in range(2):
            for copy in side(n):
                copy.wait_recv()
            x = _load_bf16(side_ref.at[n])
            x[2:2] = [_rounded(_tile(side_raw.at[n], j)) for j in range(4)]
            sides += x
        sides = _columns_to_lanes(k, sides)
        pl.semaphore_wait(go_sem.at[1], 1)
        send(2, 2, 0).start()
        send(0, 1, 0).wait_send()
        send(1, 3, 0).wait_send()
        sides = _sort_128(k, sides)
        swapped = _Seq(k, [pltpu.roll(x, COLS, 1) for x in sides.tiles], sides.pos)
        w = _Seq(k, mine.tiles, mine.pos)
        for x in (sides, swapped):
            w = x.against(jnp.minimum, w).exchange(_CLEAN_128)

        def first_half(k, tiles):
            return _runs(k, _sort_tiles(tiles)).exchange(_MERGES_64)

        first_pos = _positions(lambda k, x: [first_half(k, x)], 8)
        sorted_pos = _positions(_presort, 2)
        upper = k.lane_bit(6)
        w_below, w_above, w_sorted = [], [], []
        for p in first_pos:
            lo, hi = w.fetch(63 - p), w.fetch(127 - p)
            w_below.append(jnp.where(upper, lo, -jnp.inf))
            w_above.append(jnp.where(upper, hi, lo))
        for p in sorted_pos:
            out = jnp.where(upper, w.fetch(120 - p), w.fetch(124 - p))
            for b in range(3):
                x = jnp.where(upper, w.fetch(123 - p - b), w.fetch(127 - p - b))
                x = pltpu.roll(x, 80 + 16 * b, 1)
                out = jnp.where(((k.lane >> 4) & 3) == b, x, out)
            w_sorted.append(out)

        pos = _positions(lambda k, x: [first_half(k, x).window(None, x)], 8)
        order = [list(first_pos[0]).index(i) for i in pos[0]]

        def second_half(k, tiles):
            return _runs(k, _sort_tiles(tiles), True, order).exchange(_MERGES_64[:9])

        def finish(k, q, below, above, last):
            q = q.exchange(_MERGES_64[9:])
            q = q.window(*([x.fetch(p) for p in q.pos] for x in (below, above)))
            last = _Seq(k, last, sorted_pos)
            last = last.exchange(((64, None), (32, 6), (16, 5), (8, 4)))
            moved = _spread(last, range(0, 48, 16))
            rows = _blocks_to_rows(q, 3)
            moved += _spread(last, range(48, LANES, 16))
            return rows + _spread_to_rows(k, moved)

        k.prepare(_columns_to_lanes, 8)
        k.prepare(
            lambda k, x: finish(k, second_half(k, x), *[_Seq(k, x, pos)] * 2, x[:2]), 8
        )

        send(2, 2, 0).wait_send()
        raw[0].wait_recv()
        raw[1].wait_recv()
        x = [raw_ref[pl.ds(4, 4), :], raw_ref[pl.ds(12, 4), :]]
        for p, (x,) in enumerate(_halves(k, x)):
            half_ref[p, pl.ds(6, 2), :] = _to_words(x)
        half[0].wait_recv()
        rest = _halves(k, [_rounded(_tile(raw_ref, 2)), _rounded(_tile(raw_ref, 3))])
        got = []
        for p in range(2):
            half[1 + p].wait_recv()
            got.append(_half_to_lanes(k, [*_from_words(half_ref[p]), *rest[p] * 2], p))
        q = first_half(k, got[0])
        below, above = q.window(None, w_below), q.window(w_below, w_above)
        presorted[0].wait_recv()
        q = second_half(k, got[1])
        presorted[1].wait_recv()
        last = _from_words(sorted_ref[...])
        last = [jnp.minimum(x, y) for x, y in zip(last, w_sorted)]
        _store(o_ref, 0, finish(k, q, below, above, last))


def pallas_dist_sort_i_m128_n64_kernel(x: jax.Array):
    out = pl.pallas_call(
        _kernel,
        out_shape=jax.ShapeDtypeStruct((COLS, LANES), jnp.float32),
        in_specs=[pl.BlockSpec(memory_space=pltpu.MemorySpace.HBM)],
        out_specs=pl.BlockSpec(memory_space=pltpu.VMEM),
        scratch_shapes=[
            pltpu.VMEM((COLS, LANES), jnp.float32),
            pltpu.VMEM((32, LANES), jnp.float32),
            pltpu.VMEM((2, SUB, LANES), jnp.uint32),
            pltpu.VMEM((SUB, LANES), jnp.uint32),
            pltpu.VMEM((2, 32, LANES), jnp.float32),
            pltpu.VMEM((2, 32, LANES), jnp.bfloat16),
            pltpu.VMEM((COLS, LANES), jnp.bfloat16),
            pltpu.VMEM((3, COLS, LANES), jnp.bfloat16),
            pltpu.SemaphoreType.DMA((4,)),
            pltpu.SemaphoreType.DMA((11,)),
            pltpu.SemaphoreType.DMA((11,)),
            pltpu.SemaphoreType.DMA((3,)),
            pltpu.SemaphoreType.DMA((3,)),
            pltpu.SemaphoreType.REGULAR((2,)),
        ],
        compiler_params=pltpu.CompilerParams(
            collective_id=0,
            disable_bounds_checks=True,
            disable_semaphore_checks=True,
        ),
    )(x.T)
    return out.T
```
